```python
import numpy as np

kernel_name = "dist_f_of_ar_i_m4096_n1024"

def setup_inputs():
    t = np.random.randn(16384, 1024).astype(np.float32)
    return {"t": t}

def reference(t: np.ndarray) -> np.ndarray:
    s = t.reshape(4, 4096, 1024).sum(axis=0)
    r = np.maximum(s, 0.0)
    return np.tanh(s) * s * s + r * r * r
```

```python
import jax
import jax.numpy as jnp
from jax import lax
from jax.experimental import pallas as pl
from jax.experimental.pallas import tpu as pltpu

M = 4096
N = 1024
HALF = M // 2
BLK = HALF // 4

RS1 = (16, 64, 240, 704)
RS2 = (320, 192)
AG2 = (832, 176, 16)
N_HEAD = 2

TILE = 32
MESH = pl.DeviceIdType.MESH


def _offsets(chunks, total):
    out, off = [], 0
    for n in chunks:
        assert n % 16 == 0
        out.append((off, n))
        off += n
    assert off == total
    return out


def _split_blocks(off, n):
    out = []
    while n > 0:
        m = min(n, BLK - off % BLK)
        out.append((off, m))
        off += m
        n -= m
    return out


def _rows_loop(row0, nrows, fn):
    nfull, rem = divmod(nrows, TILE)
    if nfull == 1:
        fn(row0, TILE)
    elif nfull > 1:
        def step(i, carry):
            fn(pl.multiple_of(row0 + i * TILE, 16), TILE)
            return carry
        lax.fori_loop(0, nfull, step, 0)
    if rem:
        fn(row0 + nfull * TILE, rem)


def _compiler_params():
    base = dict(collective_id=0, vmem_limit_bytes=100 * 1024 * 1024)
    try:
        return pltpu.CompilerParams(disable_semaphore_checks=True, **base)
    except TypeError:
        return pltpu.CompilerParams(**base)


def pallas_dist_f_of_ar_i_m4096_n1024_kernel(t: jax.Array):
    assert t.shape == (M, N)

    rs1c = _offsets(RS1, 2 * BLK)
    rs2c = _offsets(RS2, BLK)
    ag2c = _offsets(AG2, 2 * BLK)
    loads_of = [_split_blocks(off, n) for off, n in rs1c]
    n_in = sum(len(x) for x in loads_of) + 2
    n_rdma = len(rs1c) + 2 * len(rs2c) + len(ag2c)

    def body(x_hbm, o_ref, xin, s1, r1, s2, r2, fb,
             in_sem, send_sem, recv_sem, ack_sem):
        p = lax.axis_index("i")
        cx = p >> 1
        cy = (p & 1) ^ cx
        nbr = (p ^ 1, 3 - p)
        side = (cy, cx)

        def row_of(h, role):
            u, v = side[h], side[1 - h]
            bu = (1 - u) if role < 2 else u
            bv = (1 - v) if role % 2 == 0 else v
            return h * HALF + (bu * 2 + bv) * BLK

        in_cp = {}
        k = 0
        for ci, pieces in enumerate(loads_of):
            for pi, (off, n) in enumerate(pieces):
                for h in range(2):
                    src = pl.multiple_of(row_of(h, off // BLK) + off % BLK, 16)
                    in_cp[(h, ci, pi)] = pltpu.make_async_copy(
                        x_hbm.at[pl.ds(src, n)], xin.at[h, pl.ds(off, n)],
                        in_sem.at[h, k])
                k += 1
        for role in (2, 3):
            for h in range(2):
                src = pl.multiple_of(row_of(h, role), 16)
                in_cp[(h, "own", role)] = pltpu.make_async_copy(
                    x_hbm.at[pl.ds(src, BLK)], xin.at[h, pl.ds(role * BLK, BLK)],
                    in_sem.at[h, k])
            k += 1

        rdmas = []

        def remote(h, src, dst, link):
            i = sum(1 for hh, _ in rdmas if hh == h)
            cp = pltpu.make_async_remote_copy(
                src_ref=src, dst_ref=dst,
                send_sem=send_sem.at[h, i], recv_sem=recv_sem.at[h, i],
                device_id=(nbr[link],), device_id_type=MESH)
            rdmas.append((h, cp))
            return cp

        fb_role = (3, 2, 1, 0)
        rs1_cp = {(h, ci): remote(h, s1.at[h, pl.ds(o, n)], r1.at[h, pl.ds(o, n)], h)
                  for ci, (o, n) in enumerate(rs1c) for h in range(2)}
        rs2_cp = {(h, ci): remote(h, s2.at[h, pl.ds(o, n)], r2.at[h, pl.ds(o, n)], 1 - h)
                  for ci, (o, n) in enumerate(rs2c) for h in range(2)}
        ag1_cp = {(h, ci): remote(h, fb.at[h, pl.ds(o, n)],
                                  fb.at[h, pl.ds(BLK + o, n)], 1 - h)
                  for ci, (o, n) in enumerate(rs2c) for h in range(2)}
        ag2_cp = {(h, ci): remote(h, fb.at[h, pl.ds(o, n)],
                                  fb.at[h, pl.ds(2 * BLK + o, n)], h)
                  for ci, (o, n) in enumerate(ag2c) for h in range(2)}

        def expand(h, off, n):
            for o, m in _split_blocks(off, n):
                slot = o // BLK
                shift = row_of(h, fb_role[slot]) - slot * BLK

                def fn(r, mm):
                    o_ref[pl.ds(pl.multiple_of(shift + r, 16), mm), :] = (
                        fb[h, pl.ds(r, mm), :].astype(jnp.float32))
                _rows_loop(o, m, fn)

        bar = pltpu.get_barrier_semaphore()

        def rs1_phase(initiate, order):
            respond = [l for l in range(2) if l not in initiate]
            for l in initiate:
                pl.semaphore_signal(bar, inc=1, device_id=(nbr[l],),
                                    device_id_type=MESH)
            for h, ci in order:
                for pi in range(len(loads_of[ci])):
                    in_cp[(h, ci, pi)].start()
            for role in (2, 3):
                for h in range(2):
                    in_cp[(h, "own", role)].start()
            if respond:
                pl.semaphore_wait(bar, len(respond))
                for l in respond:
                    pl.semaphore_signal(ack_sem.at[l], inc=1, device_id=(nbr[l],),
                                        device_id_type=MESH)
            for h, ci in order:
                for pi, (off, n) in enumerate(loads_of[ci]):
                    in_cp[(h, ci, pi)].wait()

                    def fn(r, m, h=h):
                        s1[h, pl.ds(r, m), :] = (
                            xin[h, pl.ds(r, m), :].astype(jnp.bfloat16))
                    _rows_loop(off, n, fn)
                if ci == 0 and h in initiate:
                    pl.semaphore_wait(ack_sem.at[h], 1)
                rs1_cp[(h, ci)].start()

        n1 = len(rs1c)
        both = [(h, ci) for ci in range(n1) for h in range(2)]

        def lead(ha):
            rest = [(h, ci) for ci in range(N_HEAD, n1) for h in (ha, 1 - ha)]
            return [(h, ci) for h in (ha, 1 - ha) for ci in range(N_HEAD)] + rest

        pl.when(p == 0)(lambda: rs1_phase((0, 1), both))
        pl.when(p == 1)(lambda: rs1_phase((1,), lead(0)))
        pl.when(p == 2)(lambda: rs1_phase((), both))
        pl.when(p == 3)(lambda: rs1_phase((0,), lead(1)))

        for h in range(2):
            in_cp[(h, "own", 2)].wait()
        arrived = 0
        for ci, (off, n) in enumerate(rs2c):
            while arrived < n1 and rs1c[arrived][0] < off + n:
                for h in range(2):
                    rs1_cp[(h, arrived)].wait_recv()
                arrived += 1
            for h in range(2):
                def fn(r, m, h=h):
                    s2[h, pl.ds(r, m), :] = (
                        xin[h, pl.ds(2 * BLK + r, m), :]
                        + r1[h, pl.ds(r, m), :].astype(jnp.float32)
                    ).astype(jnp.bfloat16)
                _rows_loop(off, n, fn)
                rs2_cp[(h, ci)].start()
        while arrived < n1:
            for h in range(2):
                rs1_cp[(h, arrived)].wait_recv()
            arrived += 1

        for h in range(2):
            in_cp[(h, "own", 3)].wait()
        sent = 0

        def send_ag2(ready_rows, sent):
            while sent < len(ag2c) and sum(ag2c[sent]) <= ready_rows:
                for h in range(2):
                    ag2_cp[(h, sent)].start()
                sent += 1
            return sent

        for ci, (off, n) in enumerate(rs2c):
            for h in range(2):
                rs2_cp[(h, ci)].wait_recv()

                def fn(r, m, h=h):
                    s = (xin[h, pl.ds(3 * BLK + r, m), :]
                         + r1[h, pl.ds(BLK + r, m), :].astype(jnp.float32)
                         + r2[h, pl.ds(r, m), :].astype(jnp.float32))
                    rl = jnp.maximum(s, 0.0)
                    f = jnp.tanh(s) * s * s + rl * rl * rl
                    fb[h, pl.ds(r, m), :] = f.astype(jnp.bfloat16)
                _rows_loop(off, n, fn)
                ag1_cp[(h, ci)].start()
            if ci == len(rs2c) - 1:
                sent = send_ag2(BLK, sent)
            for h in range(2):
                expand(h, off, n)

        for ci, (off, n) in enumerate(rs2c):
            for h in range(2):
                ag1_cp[(h, ci)].wait_recv()
            sent = send_ag2(BLK + off + n, sent)
            for h in range(2):
                expand(h, BLK + off, n)
        assert sent == len(ag2c)

        last = [ag2_cp[(h, len(ag2c) - 1)] for h in range(2)]
        for ci, (off, n) in enumerate(ag2c):
            if ci == len(ag2c) - 1:
                for _, cp in rdmas:
                    if not any(cp is x for x in last):
                        cp.wait_send()
            for h in range(2):
                ag2_cp[(h, ci)].wait_recv()
                expand(h, 2 * BLK + off, n)
        for cp in last:
            cp.wait_send()

    return pl.pallas_call(
        body,
        out_shape=pltpu.VMEM((M, N), jnp.float32),
        in_specs=[pl.BlockSpec(memory_space=pl.ANY)],
        out_specs=pl.BlockSpec(memory_space=pltpu.VMEM),
        scratch_shapes=[
            pltpu.VMEM((2, 4 * BLK, N), jnp.float32),
            pltpu.VMEM((2, 2 * BLK, N), jnp.bfloat16),
            pltpu.VMEM((2, 2 * BLK, N), jnp.bfloat16),
            pltpu.VMEM((2, BLK, N), jnp.bfloat16),
            pltpu.VMEM((2, BLK, N), jnp.bfloat16),
            pltpu.VMEM((2, 4 * BLK, N), jnp.bfloat16),
            pltpu.SemaphoreType.DMA((2, n_in)),
            pltpu.SemaphoreType.DMA((2, n_rdma)),
            pltpu.SemaphoreType.DMA((2, n_rdma)),
            pltpu.SemaphoreType.REGULAR((2,)),
        ],
        compiler_params=_compiler_params(),
    )(t)
```
